```python
import numpy as np

kernel_name = "dist_sort_i_m128_n64"

def setup_inputs():
    return {"x": np.random.randn(512, 64).astype(np.float32)}

def reference(x: np.ndarray) -> np.ndarray:
    return np.sort(x, axis=0)
```

```python
import numpy as np

import jax
import jax.numpy as jnp
from jax import lax
from jax.experimental import pallas as pl
from jax.experimental.pallas import tpu as pltpu

_F32 = jnp.float32
_U32 = jnp.uint32
_SORT8 = (
    (0, 2), (1, 3), (4, 6), (5, 7), (0, 4), (1, 5), (2, 6), (3, 7),
    (0, 1), (2, 3), (4, 5), (6, 7), (2, 4), (3, 5), (1, 4), (3, 6),
    (1, 2), (3, 4), (5, 6),
)


class _Ctx:
    def __init__(self):
        self.sub = lax.broadcasted_iota(jnp.int32, (8, 128), 0)
        self.lane = lax.broadcasted_iota(jnp.int32, (8, 128), 1)
        self._memo = {}

    def memo(self, key, fn):
        if key not in self._memo:
            self._memo[key] = fn()
        return self._memo[key]

    def sub_bit(self, bit):
        return self.memo(("m", bit), lambda: (self.sub & bit) != 0)

    def table(self, idx):
        idx = tuple(int(i) for i in idx)
        d = idx[0]
        if all(i == s ^ d for s, i in enumerate(idx)):
            return self.memo(("x", d), lambda: self.sub ^ d)
        word = sum(i << (3 * s) for s, i in enumerate(idx))
        return self.memo(("t", idx), lambda: (word >> (3 * self.sub)) & 7)


def _gather(v, idx):
    return jnp.take_along_axis(v, idx, axis=0, mode="promise_in_bounds")


def _permute(ctx, v, idx):
    if all(i == s for s, i in enumerate(idx)):
        return v
    return _gather(v, ctx.table(idx))


class _Seq:
    def __init__(self, vregs, pos, last):
        self.v = list(vregs)
        self.pos = np.array(pos)
        self.last = last

    def where(self):
        return {int(p): (v, s) for v, row in enumerate(self.pos) for s, p in enumerate(row)}


def _stage(ctx, seq, d, k):
    v, pos = list(seq.v), seq.pos.copy()
    at = seq.where()
    pv, ps = at[int(pos[0, 0]) ^ d]
    if pv == 0:
        bit = ps & -ps
        mask, hit = ctx.sub_bit(bit), (np.arange(8) & bit) != 0
        for a in range(len(v)):
            if not (seq.pos[a, 0] >> seq.last) & 1:
                b = at[int(seq.pos[a, 0]) ^ (1 << seq.last)][0]
                v[a] = jnp.where(mask, seq.v[b], seq.v[a])
                v[b] = jnp.where(mask, seq.v[a], seq.v[b])
                pos[a] = np.where(hit, seq.pos[b], seq.pos[a])
                pos[b] = np.where(hit, seq.pos[a], seq.pos[b])
        at = _Seq(v, pos, 0).where()
    done = set()
    for a in range(len(v)):
        b = at[int(pos[a, 0]) ^ d][0]
        if a in done or (pos[a, 0] >> seq.last) & 1 > (pos[b, 0] >> seq.last) & 1:
            continue
        done |= {a, b}
        partner = [at[int(p) ^ d] for p in pos[a]]
        assert all(pb == b for pb, _ in partner)
        other = _permute(ctx, v[b], [s for _, s in partner])
        v[a], v[b] = jnp.minimum(v[a], other), jnp.maximum(v[a], other)
        low = np.where((pos[a] >> k) & 1, pos[a] ^ d, pos[a])
        pos[a], pos[b] = low, low ^ d
    assert len(done) == len(v)
    return _Seq(v, pos, k)


def _clean(ctx, seq, top):
    for k in range(top, -1, -1):
        seq = _stage(ctx, seq, 1 << k, k)
    return seq


def _sort64(ctx, vregs):
    v = list(vregs)
    for a, b in _SORT8:
        v[a], v[b] = jnp.minimum(v[a], v[b]), jnp.maximum(v[a], v[b])
    seq = _Seq(v, np.arange(8)[:, None] + 8 * np.arange(8)[None, :], 0)
    for m in (3, 4, 5):
        seq = _clean(ctx, _stage(ctx, seq, (2 << m) - 1, m), m - 1)
    return seq


def _take(ctx, seq, want):
    at = seq.where()
    out = []
    for row in want:
        src = [at[int(p)] for p in row]
        acc = None
        for v in sorted({v for v, _ in src}):
            part = _permute(ctx, seq.v[v], [s for _, s in src])
            if acc is not None:
                word = sum(1 << i for i, (w, _) in enumerate(src) if w == v)
                mask = ctx.memo(("w", word), lambda: ((word >> ctx.sub) & 1) != 0)
                part = jnp.where(mask, part, acc)
            acc = part
        out.append(acc)
    return out


def _merge(ctx, a, b):
    n = a.pos.size
    both = _Seq(a.v + b.v, np.concatenate([a.pos, b.pos + n]), 0)
    m = n.bit_length() - 1
    return _clean(ctx, _stage(ctx, both, 2 * n - 1, m), m - 1)


def _layout(n, j):
    v, s = np.arange(n // 8)[:, None], np.arange(8)[None, :]
    return (v >> j << (j + 3)) + (s << j) + (v & ((1 << j) - 1))


def _lowest128(ctx, a, b):
    rev = _take(ctx, b, 127 - a.pos)
    return _clean(ctx, _Seq([jnp.minimum(p, q) for p, q in zip(a.v, rev)], a.pos, 0), 6)


def _lowest128_with64(ctx, low, high, r):
    pos = 63 - r.pos
    first = [jnp.minimum(m, q) for m, q in zip(low, r.v)]
    second = [jnp.maximum(m, jnp.minimum(h, q)) for m, h, q in zip(low, high, r.v)]
    return _clean(ctx, _Seq(first + second, np.concatenate([pos, pos + 64]), 0), 5)


def _shift_vregs(vregs, amount, bits, count=None):
    n = len(vregs)
    need = [set(range(count or n))]
    for bit in reversed(bits):
        need.append(need[-1] | {(u + bit) % n for u in need[-1]})
    cur = dict(enumerate(vregs))
    for bit, keep in zip(bits, reversed(need[:-1])):
        mask = (amount & bit) != 0
        cur = {u: jnp.where(mask, cur[(u + bit) % n], cur[u]) for u in sorted(keep)}
    return [cur[u] for u in sorted(cur)]


def _skew32(ctx, rows):
    t = ctx.lane + ctx.sub
    idx = t & 7
    return _shift_vregs([_gather(r, idx) for r in rows], t >> 3, (1, 2))


def _spread(ctx, lo, hi, first):
    out = []
    for u, (a, b) in enumerate(zip(lo, hi)):
        r = first + 8 * u
        mask = ((ctx.lane + ctx.sub + r) & 32) != 0
        even, odd = jnp.where(mask, b, a), jnp.where(mask, a, b)
        for k, src in enumerate((even, odd, even, odd)):
            out.append(pltpu.roll(src, r + 32 * k, 1, stride=1, stride_axis=0))
    return out


def _write_out(ctx, seq, o_ref):
    spread = int(np.bitwise_or.reduce(seq.pos[0] ^ seq.pos[0, 0]))
    j = (spread & -spread).bit_length() - 1
    lows, highs = 1 << j, 8 >> j
    at = seq.where()
    srcs = [[at[int(p)] for p in row] for row in _layout(128, j)]
    assert all(src == [(src[0][0], s) for _, s in srcs[0]] for src in srcs)
    word = sum(s << (3 * i) for i, (_, s) in enumerate(srcs[0]))
    v = [seq.v[src[0][0]] for src in srcs]
    low_bits = [1 << i for i in range(j)]
    high_bits = [1 << i for i in range(3 - j)]

    v = [_shift_vregs(v[u * lows:(u + 1) * lows], ctx.lane, low_bits) for u in range(2 * highs)]
    rows = [[None] * lows for _ in range(highs)]
    for b in range(lows):
        t = ((ctx.lane + b) >> j) + ctx.sub
        idx = (word >> (3 * (t & 7))) & 7
        mixed = [_gather(group[b], idx) for group in v]
        for u, w in enumerate(_shift_vregs(mixed, t >> 3, [highs] + high_bits[::-1], highs)):
            rows[u][b] = pltpu.roll(w, (u << (j + 3)) + b, 1, stride=lows, stride_axis=0)

    rows = [_shift_vregs(group, ctx.lane, low_bits) for group in rows]
    for b in range(lows):
        t = ((ctx.lane - b) >> j) - ctx.sub
        cols = _shift_vregs([_gather(group[-b % lows], t & 7) for group in rows], t >> 3, high_bits)
        for u in range(highs):
            first = (u << (j + 3)) + b
            o_ref[pl.ds(first, 8, stride=lows) if j else pl.ds(first, 8), :] = cols[-u % highs]


def _pack(lo, hi):
    return pltpu.bitcast(jnp.concatenate([lo, hi], axis=0).astype(jnp.bfloat16), _U32)


def _unpack(w):
    both = pltpu.bitcast(w, jnp.bfloat16).astype(_F32)
    return [both[:8], both[8:]]


def _store_run(ctx, seq, ref):
    v = _take(ctx, seq, _layout(128, 2))
    upper = ctx.lane >= 64
    for b in range(4):
        pair = [jnp.where(upper, v[b + 8 + h], v[b + h]) for h in (0, 4)]
        lo, hi = (lax.bitcast_convert_type(p, _U32) >> 16 for p in _unpack(_pack(*pair)))
        ref[pl.ds(b, 8, stride=4), :] = lo | (hi << 16)


def _load_run(ctx, ref):
    upper = ctx.lane >= 64
    v = [None] * 16
    for u in range(4):
        w = ref[pl.ds(8 * u, 8), :]
        swapped = pltpu.roll(w, 64, 1)
        for h, word in ((0, jnp.where(upper, swapped, w)), (8, jnp.where(upper, w, swapped))):
            v[u + h] = lax.bitcast_convert_type(word << 16, _F32)
            v[u + h + 4] = lax.bitcast_convert_type(word & np.uint32(0xFFFF0000), _F32)
    return _Seq(v, _layout(128, 0), 0)


def _rows(ref, first, count):
    return [ref[pl.ds(first + 8 * u, 8), :] for u in range(count)]


def _body(x_hbm, o_ref, xv, runs, raw, msg, load_sems, send_sems, recv_sems, go):
    me = lax.axis_index("i")
    barrier = pltpu.get_barrier_semaphore()

    def signal(sem, dev):
        pl.semaphore_signal(sem, 1, device_id=dev, device_id_type=pl.DeviceIdType.LOGICAL)

    def remote(src, dst, send, recv, dev):
        return pltpu.make_async_remote_copy(
            src, dst, send_sems.at[send], recv_sems.at[recv],
            device_id=dev, device_id_type=pl.DeviceIdType.LOGICAL)

    def run_copy(src, dst):
        return remote(runs.at[src], runs.at[src], dst, src, dst)

    def raw_copy():
        return remote(x_hbm.at[pl.ds(0, 32)], raw, 0, 2, 0)

    def msg_copy(j):
        return remote(msg.at[j], msg.at[j], 4 + j, 4 + j, 0)

    def load(j):
        rows = pl.ds(32 * j, 32)
        return pltpu.make_async_copy(x_hbm.at[rows], xv.at[rows], load_sems.at[j])

    load(1).start()

    @pl.when(me == 2)
    def _():
        pl.semaphore_wait(barrier, 1)
        raw_copy().start()
        signal(go.at[0], 0)
        ctx = _Ctx()
        load(1).wait()
        hi = _skew32(ctx, _rows(xv, 32, 4))
        for j in range(2):
            msg[j] = _pack(hi[2 * j], hi[2 * j + 1])
            msg_copy(j).start()

    load(0).start()

    @pl.when(me == 0)
    def _():
        for dev in (2, 1, 3):
            signal(barrier, dev)

    @pl.when(me % 2 == 1)
    def _():
        signal(barrier, 0)

    @pl.when(me != 2)
    def _():
        load(1).wait()

    load(0).wait()
    ctx = _Ctx()
    lo, hi = _skew32(ctx, _rows(xv, 0, 4)), _skew32(ctx, _rows(xv, 32, 4))
    halves = [_sort64(ctx, _spread(ctx, lo[u:u + 2], hi[u:u + 2], 8 * u)) for u in (0, 2)]
    _store_run(ctx, _merge(ctx, *halves), runs.at[me])

    @pl.when(me == 0)
    def _():
        pl.semaphore_wait(barrier, 2)
        signal(barrier, 2)
        for dev in (1, 3):
            signal(go.at[0], dev)
            run_copy(0, dev).start()
        pl.semaphore_wait(go.at[0], 1)
        for dev in (1, 3):
            signal(go.at[1], dev)
        run_copy(0, 2).start()
        ctx = _Ctx()
        best = _load_run(ctx, runs.at[0])
        for dev in (3, 1):
            run_copy(dev, 0).wait_recv()
        for dev in (3, 1):
            best = _lowest128(ctx, _load_run(ctx, runs.at[dev]), best)
        for dev in (1, 3, 2):
            run_copy(0, dev).wait_send()
        raw_copy().wait_recv()
        lo = _skew32(ctx, _rows(raw, 0, 4))
        for j in range(2):
            msg_copy(j).wait_recv()
            r = _sort64(ctx, _spread(ctx, lo[2 * j:2 * j + 2], _unpack(msg[j]), 16 * j))
            low, high = _take(ctx, best, 63 - r.pos), _take(ctx, best, 127 - r.pos)
            best = _lowest128_with64(ctx, low, high, r)
        _write_out(ctx, best, o_ref)

    @pl.when(me != 0)
    def _():
        pl.semaphore_wait(barrier, 1)

        @pl.when(me == 2)
        def _():
            run_copy(2, 3).start()
            run_copy(2, 1).start()
            raw_copy().wait_send()
            for j in range(2):
                msg_copy(j).wait_send()

        @pl.when(me != 2)
        def _():
            run_copy(me, 0).start()
            pl.semaphore_wait(go.at[0], 1)
            run_copy(me, 4 - me).start()
            pl.semaphore_wait(go.at[1], 1)
            run_copy(me, 2).start()
            run_copy(me, 0).wait_send()

        ctx = _Ctx()
        a, b = me % 3 + 1, (me + 1) % 3 + 1
        run_copy(0, me).wait_recv()
        p = _merge(ctx, _load_run(ctx, runs.at[me]), _load_run(ctx, runs.at[0]))
        run_copy(a, me).wait_recv()
        run_copy(b, me).wait_recv()
        q = _merge(ctx, _load_run(ctx, runs.at[a]), _load_run(ctx, runs.at[b]))

        def pick(upper, s, t):
            return jnp.where(upper, jnp.maximum(s, t), jnp.minimum(s, t))

        half = [pick(me >= 2, s, t) for s, t in zip(p.v, _take(ctx, q, 255 - p.pos))]
        half = _Seq(half, p.pos, 0)
        pos = p.pos[p.pos[:, 0] < 128]
        mine = [
            pick(me % 2 == 1, s, t)
            for s, t in zip(_take(ctx, half, pos), _take(ctx, half, pos + 128))
        ]
        _write_out(ctx, _clean(ctx, _Seq(mine, pos, 0), 6), o_ref)
        run_copy(me, a).wait_send()
        run_copy(me, b).wait_send()


def pallas_dist_sort_i_m128_n64_kernel(x: jax.Array):
    xt = x.T
    out = pl.pallas_call(
        _body,
        out_shape=jax.ShapeDtypeStruct(xt.shape, _F32),
        in_specs=[pl.BlockSpec(memory_space=pltpu.HBM)],
        out_specs=pl.BlockSpec(memory_space=pltpu.VMEM),
        scratch_shapes=[
            pltpu.VMEM((64, 128), _F32),
            pltpu.VMEM((4, 32, 128), _U32),
            pltpu.VMEM((32, 128), _F32),
            pltpu.VMEM((2, 8, 128), _U32),
            pltpu.SemaphoreType.DMA((2,)),
            pltpu.SemaphoreType.DMA((6,)),
            pltpu.SemaphoreType.DMA((6,)),
            pltpu.SemaphoreType.REGULAR((2,)),
        ],
        compiler_params=pltpu.CompilerParams(
            collective_id=0,
            disable_bounds_checks=True,
            disable_semaphore_checks=True,
        ),
    )(xt)
    return out.T
```

```python
import numpy as np

import jax
import jax.numpy as jnp
from jax import lax
from jax.experimental import pallas as pl
from jax.experimental.pallas import tpu as pltpu

_F32 = jnp.float32
_U32 = jnp.uint32
_RAW = 28
_REST = (32 - _RAW) // 2


def _or_none(fn):
    return lambda *args: None if any(a is None for a in args) else fn(*args)


_min, _max, _where = map(_or_none, (jnp.minimum, jnp.maximum, jnp.where))


@_or_none
def _gather(v, idx):
    dims = lax.GatherDimensionNumbers(
        offset_dims=(), collapsed_slice_dims=(0,), start_index_map=(0,),
        operand_batching_dims=(1,), start_indices_batching_dims=(1,))
    return lax.gather(
        v, idx.reshape(8, 128, 1), dims, (1, 1), mode=lax.GatherScatterMode.PROMISE_IN_BOUNDS)


class _Ctx:
    def __init__(self):
        self.sub = lax.broadcasted_iota(jnp.int32, (8, 128), 0)
        self.lane = lax.broadcasted_iota(jnp.int32, (8, 128), 1)
        self._memo = {}

    def memo(self, key, fn):
        if key not in self._memo:
            self._memo[key] = fn()
        return self._memo[key]

    def sub_bit(self, bit):
        return self.memo(("sub", bit), lambda: (self.sub & bit) != 0)

    def lane_bit(self, bit):
        return self.memo(("lane", bit), lambda: (self.lane & bit) != 0)

    def permute(self, v, idx):
        idx = tuple(idx)
        if idx == tuple(range(8)):
            return v
        if all(i == s ^ idx[0] for s, i in enumerate(idx)):
            return _gather(v, self.memo(idx, lambda: self.sub ^ idx[0]))
        word = sum(i << (3 * s) for s, i in enumerate(idx))
        return _gather(v, self.memo(idx, lambda: (word >> (3 * self.sub)) & 7))


class _Seq:
    def __init__(self, vregs, pos, last=0):
        self.v = list(vregs)
        self.pos = np.array(pos)
        self.last = last

    def where(self):
        return {int(p): (v, s) for v, row in enumerate(self.pos) for s, p in enumerate(row)}


def _layout(n, j):
    v, s = np.arange(n // 8)[:, None], np.arange(8)[None, :]
    return (v >> j << (j + 3)) + (s << j) + (v & ((1 << j) - 1))


def _trade(ctx, seq, d):
    v, pos, at = list(seq.v), seq.pos.copy(), seq.where()
    step = at[int(pos[0, 0]) ^ d][1]
    bit = step & -step
    mask, hit = ctx.sub_bit(bit), (np.arange(8) & bit) != 0
    for a in range(len(v)):
        b = at[int(seq.pos[a, 0]) ^ (1 << seq.last)][0]
        v[a] = _where(mask, seq.v[b], seq.v[a])
        pos[a] = np.where(hit, seq.pos[b], seq.pos[a])
    return _Seq(v, pos, seq.last)


def _stage(ctx, seq, d, k, flip=False):
    if seq.where()[int(seq.pos[0, 0]) ^ d][0] == 0:
        seq = _trade(ctx, seq, d)
    v, pos, at = list(seq.v), seq.pos.copy(), seq.where()
    side = (seq.pos[:, 0] >> seq.last) & 1
    for a in range(len(v)):
        partner = [at[int(p) ^ d] for p in seq.pos[a]]
        b = partner[0][0]
        assert all(w == b for w, _ in partner)
        if ((side[a], a) < (side[b], b)) != flip:
            other = ctx.permute(seq.v[b], [s for _, s in partner])
            v[a], v[b] = _min(seq.v[a], other), _max(seq.v[a], other)
            pos[a] = np.where((seq.pos[a] >> k) & 1, seq.pos[a] ^ d, seq.pos[a])
            pos[b] = pos[a] ^ d
    return _Seq(v, pos, k)


def _clean(ctx, seq, top, flip=False):
    for k in range(top, -1, -1):
        seq = _stage(ctx, seq, 1 << k, k, flip)
    return seq


def _merge_vregs(a, b):
    if not a or not b:
        return a + b
    if len(a) == len(b) == 1:
        return [_min(a[0], b[0]), _max(a[0], b[0])]
    even, odd = _merge_vregs(a[::2], b[::2]), _merge_vregs(a[1::2], b[1::2])
    out = even[:1]
    for i, v in enumerate(odd):
        out += _merge_vregs([v], even[i + 1:i + 2])
    return out + even[len(odd) + 1:]


def _sort_vregs(v):
    half = len(v) // 2
    return _merge_vregs(_sort_vregs(v[:half]), _sort_vregs(v[half:])) if half else v


def _presort(v):
    first = _merge_vregs(_sort_vregs([v[4], v[5], v[0], v[2]]), _sort_vregs([v[1], v[3]]))
    return first, _sort_vregs(v[6:])


def _merge_sublanes(ctx, v, levels=3):
    n = len(v)
    seq = _Seq(v, np.arange(n)[:, None] + n * np.arange(8)[None, :])
    for m in range(n.bit_length() - 1, n.bit_length() - 1 + levels):
        seq = _clean(ctx, _stage(ctx, seq, (2 << m) - 1, m), m - 1)
    return seq


def _take(ctx, seq, want):
    at = seq.where()
    out = []
    for row in want:
        src = [at[int(p)] for p in row]
        first, *others = sorted({v for v, _ in src})
        acc = ctx.permute(seq.v[first], [s for _, s in src])
        for v in others:
            word = sum(1 << i for i, (w, _) in enumerate(src) if w == v)
            part = ctx.permute(seq.v[v], [s for _, s in src])
            acc = _where(ctx.memo(word, lambda: ((word >> ctx.sub) & 1) != 0), part, acc)
        out.append(acc)
    return out


def _keep_half(ctx, seq, upper):
    n = seq.pos.size // 2
    pos = seq.pos[seq.pos[:, 0] < n]
    pairs = zip(_take(ctx, seq, pos), _take(ctx, seq, pos + n))
    return _Seq([_where(upper, t, s) for s, t in pairs], pos)


def _join(a, b):
    return _Seq(a.v + b.v, np.concatenate([a.pos, b.pos + a.pos.size]))


def _lowest(ctx, a, b):
    pairs = zip(a.v, _take(ctx, b, 127 - a.pos))
    return _clean(ctx, _Seq([_min(s, t) for s, t in pairs], a.pos), 6)


def _window(ctx, blocks, run):
    assert (run.pos[:4] + 32 == run.pos[4:]).all()
    out = []
    for u in range(4):
        low = _max(blocks[1][u], run.v[u])
        high = _max(blocks[2][u], run.v[u + 4]) if len(blocks) > 2 else run.v[u + 4]
        out.append(_min(_min(low, high), blocks[0][u]))
    return _clean(ctx, _Seq(out, 31 - run.pos[:4]), 4, True)


def _shift_masks(amount, n):
    return [(bit, (amount & bit) != 0) for bit in (1, 2, 4) if bit < n]


def _shift_vregs(vregs, masks):
    n = len(vregs)
    for bit, mask in masks:
        vregs = [_where(mask, vregs[(u + bit) % n], vregs[u]) for u in range(n)]
    return vregs


def _skewer(ctx, n):
    t = ctx.lane + ctx.sub
    idx, masks = t & 7, _shift_masks(t >> 3, n // 8)
    return lambda rows: _shift_vregs([_gather(r, idx) for r in rows], masks)


def _spread(rows, first, turns):
    return [
        pltpu.roll(v, first + 8 * u + k, 1, stride=1, stride_axis=0)
        for u, v in enumerate(rows) for k in turns
    ]


def _sort_shard(ctx, rows):
    return _merge_sublanes(ctx, _sort_vregs(_spread(_skewer(ctx, 64)(rows), 0, (0, 64))))


def _writer(ctx, pos):
    n = pos.size
    spread = int(np.bitwise_or.reduce(pos[0] ^ pos[0, 0]))
    j = (spread & -spread).bit_length() - 1
    lows, highs = 1 << j, n // 8 >> j
    at = _Seq([], pos).where()
    srcs = [[at[int(p)] for p in row] for row in _layout(n, j)]
    assert all(src == [(src[0][0], s) for _, s in srcs[0]] for src in srcs)
    word = sum(s << (3 * i) for i, (_, s) in enumerate(srcs[0]))
    low_masks = _shift_masks(ctx.lane, lows)
    ups = [((ctx.lane + b) >> j) + ctx.sub for b in range(lows)]
    ups = [((word >> (3 * (t & 7))) & 7, _shift_masks(t >> 3, highs)) for t in ups]
    downs = [((ctx.lane - b) >> j) - ctx.sub for b in range(lows)]
    downs = [(t & 7, _shift_masks(t >> 3, highs)) for t in downs]
    room = (ctx.lane & (n - 1)) - (ctx.sub << j)

    def write(vregs, put):
        v = [vregs[src[0][0]] for src in srcs]
        v = [_shift_vregs(v[u * lows:(u + 1) * lows], low_masks) for u in range(highs)]
        rows = [[None] * lows for _ in range(highs)]
        for b, (idx, masks) in enumerate(ups):
            for u, w in enumerate(_shift_vregs([_gather(group[b], idx) for group in v], masks)):
                r = (u << (j + 3)) + b
                plain, wrapped = (
                    pltpu.roll(w, r + k, 1, stride=lows, stride_axis=0) for k in (0, 128 - n))
                rows[u][b] = _where(room < r, wrapped, plain)
        rows = [_shift_vregs(group, low_masks) for group in rows]
        for b, (idx, masks) in enumerate(downs):
            cols = _shift_vregs([_gather(group[-b % lows], idx) for group in rows], masks)
            for u in range(highs):
                put((u << (j + 3)) + b, lows, cols[-u % highs])

    return write


def _pack(lo, hi):
    lo, hi = (lax.bitcast_convert_type(v, _U32) + np.uint32(0x8000) for v in (lo, hi))
    return (lo >> 16) | (hi & np.uint32(0xFFFF0000))


def _unpack(w):
    return [lax.bitcast_convert_type(h, _F32) for h in (w << 16, w & np.uint32(0xFFFF0000))]


def _store_run(ctx, seq, ref):
    v = _take(ctx, _keep_half(ctx, seq, ctx.lane_bit(64)), _layout(64, 1))
    for u in range(4):
        ref[pl.ds(16 * (u >> 1) + (u & 1), 8, stride=2), :] = _pack(v[u], v[u + 4])


def _load_run(ctx, ref):
    v = [None] * 16
    for u in range(4):
        w = ref[pl.ds(8 * u, 8), :]
        swapped = pltpu.roll(w, 64, 1)
        v[u], v[u + 4] = _unpack(_where(ctx.lane_bit(64), swapped, w))
        v[u + 8], v[u + 12] = _unpack(_where(ctx.lane_bit(64), w, swapped))
    return _Seq(v, _layout(128, 0))


def _rows(ref, first, count):
    return [ref[pl.ds(first + 8 * u, 8), :] for u in range(count)]


def _body(x_hbm, o_ref, xv, side, runs, raw, msg, held, load_sems, send_sems, recv_sems, go):
    barrier = pltpu.get_barrier_semaphore()
    rest = pl.ds(8 - _REST, _REST)

    def signal(sem, dev):
        pl.semaphore_signal(sem, 1, device_id=dev, device_id_type=pl.DeviceIdType.LOGICAL)

    def remote(src, dst, send, recv, dev):
        return pltpu.make_async_remote_copy(
            src, dst, send_sems.at[send], recv_sems.at[recv],
            device_id=dev, device_id_type=pl.DeviceIdType.LOGICAL)

    def run_copy(src, dst):
        return remote(runs.at[src], runs.at[src], dst, src, dst)

    def side_copy():
        return remote(x_hbm, side, 0, 1, 0)

    def raw_copy():
        return remote(x_hbm.at[pl.ds(0, _RAW)], raw.at[pl.ds(0, _RAW)], 0, 2, 0)

    def msg_copy(j):
        rows = rest if j == 2 else pl.ds(0, 8)
        return remote(msg.at[j, rows], msg.at[j, rows], 4 + j, 4 + j, 0)

    def load(j):
        rows = pl.ds(_RAW, 64 - _RAW) if j else pl.ds(0, _RAW)
        return pltpu.make_async_copy(x_hbm.at[rows], xv.at[rows], load_sems.at[j])

    def put(first, stride, v):
        o_ref[pl.ds(first, 8, stride=stride), :] = v

    def put_both(first, stride, w):
        for k, v in zip((0, 32), _unpack(w)):
            put(first + k, stride, v)

    load(1).start()
    me = lax.axis_index("i")

    @pl.when(me == 2)
    def _():
        pl.semaphore_wait(barrier, 1)
        raw_copy().start()
        signal(go.at[0], 0)
        ctx = _Ctx()
        skew = _skewer(ctx, 32)
        load(1).wait()
        right = skew(_rows(xv, 32, 4))
        msg[2, rest, :] = _pack(xv[pl.ds(_RAW, _REST), :], xv[pl.ds(_RAW + _REST, _REST), :])
        msg_copy(2).start()
        msg[0] = _pack(right[0], right[1])
        msg_copy(0).start()
        late = _spread(right[2:3], 16, (0, 32, 64, 96)) + _spread(right[3:], 24, (0, 32))
        late += _spread(skew(_rows(xv, 32, 4))[3:], 24, (64, 96))
        late = _merge_sublanes(ctx, _merge_vregs(*_presort(late)), 2)
        late = _keep_half(ctx, _stage(ctx, late, 63, 5), ctx.lane_bit(64))
        late = _keep_half(ctx, _stage(ctx, late, 16, 4), ctx.lane_bit(32))
        late = _clean(ctx, late, 3)
        assert (late.pos == _merge_sublanes(ctx, [None] * 8).pos[:2]).all()
        msg[1] = _pack(*late.v)
        msg_copy(1).start()

    @pl.when(me == 1)
    def _():
        pl.semaphore_wait(barrier, 1)
        side_copy().start()

    load(0).start()

    @pl.when(me == 0)
    def _():
        for dev in (2, 1, 3):
            signal(barrier, dev)

    @pl.when((me & 1) == 1)
    def _():
        signal(barrier, 0)

    @pl.when(me != 2)
    def _():
        load(1).wait()

    load(0).wait()
    ctx = _Ctx()
    _store_run(ctx, _sort_shard(ctx, _rows(xv, 0, 8)), runs.at[me])

    @pl.when(me != 0)
    def _():
        @pl.when(me == 2)
        def _():
            pl.semaphore_wait(barrier, 1)
            run_copy(2, 3).start()
            run_copy(2, 1).start()
            raw_copy().wait_send()
            for j in range(3):
                msg_copy(j).wait_send()

        for dev in (1, 3):
            @pl.when(me == dev)
            def _():
                if dev == 3:
                    pl.semaphore_wait(barrier, 1)
                    run_copy(3, 0).start()
                pl.semaphore_wait(go.at[0], 1)
                run_copy(dev, 4 - dev).start()
                pl.semaphore_wait(go.at[1], 1)
                run_copy(dev, 2).start()
                (run_copy(3, 0) if dev == 3 else side_copy()).wait_send()

        ctx = _Ctx()

        def merge(a, b):
            both = _join(_load_run(ctx, runs.at[a]), _load_run(ctx, runs.at[b]))
            return _clean(ctx, _stage(ctx, both, 255, 7), 6)

        a, b = jnp.where(me == 1, 2, 1), jnp.where(me == 3, 2, 3)
        run_copy(0, 0).wait_recv()
        p = merge(me, 0)
        run_copy(a, 0).wait_recv()
        run_copy(b, 0).wait_recv()
        q = _Seq(_take(ctx, merge(a, b), 255 - p.pos), 255 - p.pos)
        mine = _keep_half(ctx, _stage(ctx, _join(p, q), 511, 8), me >= 2)
        mine = _keep_half(ctx, _stage(ctx, mine, 128, 7), (me & 1) == 1)
        mine = _keep_half(ctx, _stage(ctx, mine, 64, 6), ctx.lane_bit(64))
        mine = _clean(ctx, mine, 5)
        _writer(ctx, mine.pos)(mine.v, put)
        for dev in (a, b):
            remote(runs.at[me], runs.at[me], dev, 0, 0).wait_send()

    @pl.when(me == 0)
    def _():
        pl.semaphore_wait(barrier, 2)
        signal(barrier, 2)
        for dev in (1, 3):
            signal(go.at[0], dev)
            run_copy(0, dev).start()
        pl.semaphore_wait(go.at[0], 1)
        for dev in (1, 3):
            signal(go.at[1], dev)
        run_copy(0, 2).start()

        ctx = _Ctx()
        best = _load_run(ctx, runs.at[0])
        side_copy().wait_recv()
        rows = [_unpack(_pack(v, v))[1] for v in _rows(side, 0, 8)]
        best = _lowest(ctx, best, _sort_shard(ctx, rows))
        run_copy(3, 0).wait_recv()
        best = _lowest(ctx, _load_run(ctx, runs.at[3]), best)

        odd, upper = ctx.lane_bit(32), ctx.lane_bit(64)
        turned = [pltpu.roll(v, 32, 1) for v in best.v]
        late = _merge_sublanes(ctx, [None] * 8)
        first, order = _trade(ctx, late, 8).pos[:, :1], np.array([[0, 4, 2, 6, 1, 5, 3, 7]])
        early_pos = (first & ~15) + order + ((first ^ order) & 1) * 8
        floor = [jnp.full((8, 128), -jnp.inf, _F32)] * 4
        for h in range(2):
            v = [_where(odd, *(pair if h else pair[::-1])) for pair in zip(best.v, turned)]
            q = [_take(ctx, _Seq(v, best.pos), top - early_pos[:4]) for top in (127, 95, 63, 31)]
            for step, mask in ((2, upper), (1, odd)):
                q = [[_where(mask, s, t) for s, t in zip(a, b)]
                     for a, b in zip(q, q[step:] + [floor] * step)]
            for i, w in enumerate(sum(q, [])):
                held[h, pl.ds(8 * i, 8), :] = w
        write = _writer(ctx, _window(ctx, [floor] * 2, late).pos)
        skew = _skewer(ctx, 32)
        _take(ctx, _trade(ctx, late, 8), early_pos)
        for dev in (1, 3, 2):
            run_copy(0, dev).wait_send()

        def as_run(words):
            return _Seq(sum(map(_unpack, words), []), late.pos)

        def absorb(h, run):
            run = _Seq(_take(ctx, _trade(ctx, run, 8), early_pos), early_pos)
            blocks = [_rows(held.at[h], 32 * j, 4) for j in range(4)]
            return [
                _take(ctx, _window(ctx, blocks[j:j + 3], run), 31 - late.pos[:4]) for j in range(3)
            ]

        def finish(blocks, words):
            out = _window(ctx, blocks, as_run(words))
            return [lax.bitcast_convert_type(v, _U32) for v in out.v]

        raw_copy().wait_recv()
        msg_copy(2).wait_recv()
        for k, v in enumerate(_unpack(msg[2, rest, :])):
            raw[pl.ds(_RAW + k * _REST, _REST), :] = v
        left = _presort(_spread(skew(_rows(raw, 0, 4)), 0, (0, 64)))
        msg_copy(0).wait_recv()
        right = _presort(_spread(_unpack(msg[0]), 0, (0, 32, 64, 96)))
        left = _merge_sublanes(ctx, _merge_vregs(*left))
        words = [_pack(left.v[2 * g], left.v[2 * g + 1]) for g in range(4)]
        left = absorb(0, as_run(words))
        msg_copy(1).wait_recv()
        words = [pltpu.roll(w, 32, 1) for w in words]
        w = msg[1]
        turned = [w] + [pltpu.roll(w, k, 1) for k in (32, 64, 96)]
        turned = _shift_vregs(turned, [(2, upper), (1, odd)])
        right = absorb(1, _merge_sublanes(ctx, _merge_vregs(*right)))
        left, right = finish(left, words), finish(right, [turned[-g % 4] for g in range(4)])
        write([(p >> 16) | q for p, q in zip(left, right)], put_both)


def pallas_dist_sort_i_m128_n64_kernel(x: jax.Array):
    xt = x.T
    out = pl.pallas_call(
        _body,
        out_shape=jax.ShapeDtypeStruct(xt.shape, _F32),
        in_specs=[pl.BlockSpec(memory_space=pltpu.HBM)],
        out_specs=pl.BlockSpec(memory_space=pltpu.VMEM),
        scratch_shapes=[
            pltpu.VMEM((64, 128), _F32),
            pltpu.VMEM((64, 128), _F32),
            pltpu.VMEM((4, 32, 128), _U32),
            pltpu.VMEM((32, 128), _F32),
            pltpu.VMEM((3, 8, 128), _U32),
            pltpu.VMEM((2, 128, 128), _F32),
            pltpu.SemaphoreType.DMA((2,)),
            pltpu.SemaphoreType.DMA((7,)),
            pltpu.SemaphoreType.DMA((7,)),
            pltpu.SemaphoreType.REGULAR((2,)),
        ],
        compiler_params=pltpu.CompilerParams(
            collective_id=0,
            disable_bounds_checks=True,
            disable_semaphore_checks=True,
        ),
    )(xt)
    return out.T
```
